```python
import numpy as np

kernel_name = "dist_sum_ax1_xy_m512_n256"

def setup_inputs():
    return {"x": np.random.randn(1024, 512).astype(np.float32)}

def reference(x: np.ndarray) -> np.ndarray:
    return np.sum(x, axis=1, keepdims=True)
```

```python
import jax
import jax.numpy as jnp
from jax import lax
from jax.experimental import pallas as pl
from jax.experimental.pallas import tpu as pltpu


def pallas_dist_sum_ax1_xy_m512_n256_kernel(
x: jax.Array,
):
    m, n = x.shape

    def kernel_body(x_hbm, out_ref, x_vmem, part, recv, in_sem, send_sem, recv_sem):
        my_x = lax.axis_index("x")
        my_y = lax.axis_index("y")
        peer = (my_x, 1 - my_y)

        load = pltpu.make_async_copy(x_hbm, x_vmem, in_sem)
        load.start()

        barrier = pltpu.get_barrier_semaphore()
        pl.semaphore_signal(
            barrier, inc=1, device_id=peer, device_id_type=pl.DeviceIdType.MESH
        )

        load.wait()
        v = x_vmem[:, :128] + x_vmem[:, 128:]
        part[...] = jnp.sum(v.T, axis=0, keepdims=True)

        pl.semaphore_wait(barrier, 1)
        rdma = pltpu.make_async_remote_copy(
            src_ref=part,
            dst_ref=recv,
            send_sem=send_sem,
            recv_sem=recv_sem,
            device_id=peer,
            device_id_type=pl.DeviceIdType.MESH,
        )
        rdma.start()
        rdma.wait_recv()
        out_ref[...] = part[...] + recv[...]
        rdma.wait_send()

    out = pl.pallas_call(
        kernel_body,
        out_shape=jax.ShapeDtypeStruct((1, m), x.dtype),
        in_specs=[pl.BlockSpec(memory_space=pl.ANY)],
        out_specs=pl.BlockSpec(memory_space=pltpu.VMEM),
        scratch_shapes=[
            pltpu.VMEM((m, n), x.dtype),
            pltpu.VMEM((1, m), x.dtype),
            pltpu.VMEM((1, m), x.dtype),
            pltpu.SemaphoreType.DMA,
            pltpu.SemaphoreType.DMA,
            pltpu.SemaphoreType.DMA,
        ],
        compiler_params=pltpu.CompilerParams(collective_id=0),
    )(x)
    return out.reshape(m, 1)
```

```python
import jax
import jax.numpy as jnp
from jax import lax
from jax.experimental import pallas as pl
from jax.experimental.pallas import tpu as pltpu

_SUB, _LANE = 8, 128
_LOADS = (144, 112, 96, 88, 72)


def pallas_dist_sum_ax1_xy_m512_n256_kernel(
x: jax.Array,
):
    m, n = x.shape
    assert sum(_LOADS) == m and n % _LANE == 0
    n_tiles = m // _LANE

    def kernel_body(x_hbm, out_ref, x_vmem, mine, theirs, load_sems, send_sems, recv_sems):
        peer = (lax.axis_index("x"), 1 - lax.axis_index("y"))

        loads, row = [], 0
        for i, rows in enumerate(_LOADS):
            span = pl.ds(row, rows)
            load = pltpu.make_async_copy(x_hbm.at[span], x_vmem.at[span], load_sems.at[i])
            load.start()
            loads.append((row, rows, load))
            row += rows

        barrier = pltpu.get_barrier_semaphore()
        pl.semaphore_signal(barrier, 1, device_id=peer, device_id_type=pl.DeviceIdType.MESH)

        sends = [
            pltpu.make_async_remote_copy(
                src_ref=mine.at[:, pl.ds(t * _LANE, _LANE)],
                dst_ref=theirs.at[:, pl.ds(t * _LANE, _LANE)],
                send_sem=send_sems.at[t],
                recv_sem=recv_sems.at[t],
                device_id=peer,
                device_id_type=pl.DeviceIdType.MESH,
            )
            for t in range(n_tiles)
        ]

        diag = lax.broadcasted_iota(jnp.int32, (_SUB, _LANE), 1) - lax.broadcasted_iota(
            jnp.int32, (_SUB, _LANE), 0
        )
        sent = 0
        for first, rows, load in loads:
            load.wait()
            for r in range(first, first + rows, _SUB):
                v = x_vmem[pl.ds(r, _SUB), pl.ds(0, _LANE)]
                for c in range(_LANE, n, _LANE):
                    v = v + x_vmem[pl.ds(r, _SUB), pl.ds(c, _LANE)]
                if r % _LANE == 0:
                    acc = jnp.zeros((_SUB, _LANE), jnp.float32)
                acc = jnp.where(diag == r % _LANE, jnp.sum(v, axis=1, keepdims=True), acc)
                if (r + _SUB) % _LANE == 0:
                    mine[:, pl.ds(r + _SUB - _LANE, _LANE)] = jnp.sum(acc, axis=0, keepdims=True)
            while (sent + 1) * _LANE <= first + rows:
                if sent == 0:
                    pl.semaphore_wait(barrier, 1)
                sends[sent].start()
                sent += 1

        for t, send in enumerate(sends):
            if t == n_tiles - 1:
                for s in sends:
                    s.wait_send()
            send.wait_recv()
            span = pl.ds(t * _LANE, _LANE)
            out_ref[:, span] = mine[:, span] + theirs[:, span]

    out = pl.pallas_call(
        kernel_body,
        out_shape=jax.ShapeDtypeStruct((1, m), x.dtype),
        in_specs=[pl.BlockSpec(memory_space=pltpu.HBM)],
        out_specs=pl.BlockSpec(memory_space=pltpu.VMEM),
        scratch_shapes=[
            pltpu.VMEM((m, n), x.dtype),
            pltpu.VMEM((1, m), x.dtype),
            pltpu.VMEM((1, m), x.dtype),
            pltpu.SemaphoreType.DMA((len(_LOADS),)),
            pltpu.SemaphoreType.DMA((n_tiles,)),
            pltpu.SemaphoreType.DMA((n_tiles,)),
        ],
        compiler_params=pltpu.CompilerParams(
            collective_id=0,
            disable_bounds_checks=True,
            disable_semaphore_checks=True,
        ),
    )(x)
    return out.reshape(m, 1)
```

```python
import jax
import jax.numpy as jnp
from jax import lax
from jax.experimental import pallas as pl
from jax.experimental.pallas import tpu as pltpu

_SUBLANES, _LANES = 8, 128

_LAST_TILE_COPIES = (48, 16, 16, 16, 8, 8, 8, 8)

_FLAGS = (
    {"XLA_TPU_RESCHEDULE_DMA_DONES": True}
    if jax.__version_info__ >= (0, 12)
    else None
)


def pallas_dist_sum_ax1_xy_m512_n256_kernel(
x: jax.Array,
):
    m, n = x.shape
    assert m % _LANES == 0 and n % _LANES == 0
    num_tiles = m // _LANES
    tile_copies = [(_LANES,)] * (num_tiles - 1) + [_LAST_TILE_COPIES]
    num_copies = sum(len(copies) for copies in tile_copies)

    def kernel_body(
        x_hbm, out_ref, x_vmem, mine, theirs, load_sems, send_sems, recv_sems
    ):
        peer = (lax.axis_index("x"), 1 - lax.axis_index("y"))

        tile_loads, row, sem = [], 0, 0
        for copies in tile_copies:
            tile_loads.append([])
            for rows in copies:
                span = pl.ds(row, rows)
                load = pltpu.make_async_copy(
                    x_hbm.at[span], x_vmem.at[span], load_sems.at[sem]
                )
                load.start(priority=0 if row == 0 else 1)
                tile_loads[-1].append((range(row, row + rows, _SUBLANES), load))
                row, sem = row + rows, sem + 1

        barrier = pltpu.get_barrier_semaphore()
        pl.semaphore_signal(
            barrier, 1, device_id=peer, device_id_type=pl.DeviceIdType.MESH
        )

        sends = [
            pltpu.make_async_remote_copy(
                src_ref=mine.at[t],
                dst_ref=theirs.at[t],
                send_sem=send_sems.at[t],
                recv_sem=recv_sems.at[t],
                device_id=peer,
                device_id_type=pl.DeviceIdType.MESH,
            )
            for t in range(num_tiles)
        ]

        vreg = (_SUBLANES, _LANES)
        lane_minus_sublane = lax.broadcasted_iota(
            jnp.int32, vreg, 1
        ) - lax.broadcasted_iota(jnp.int32, vreg, 0)

        for t, loads in enumerate(tile_loads):
            folded = []
            for group_rows, load in loads:
                load.wait()
                for r in group_rows:
                    group = pl.ds(r, _SUBLANES)
                    v = x_vmem[group, pl.ds(0, _LANES)]
                    for c in range(_LANES, n, _LANES):
                        v = v + x_vmem[group, pl.ds(c, _LANES)]
                    folded.append(v)
            spread = jnp.zeros(vreg, x.dtype)
            for g, v in enumerate(folded):
                spread = jnp.where(
                    lane_minus_sublane == g * _SUBLANES,
                    jnp.sum(v, axis=1, keepdims=True),
                    spread,
                )
            mine[t] = jnp.sum(spread, axis=0, keepdims=True)
            if t == 0:
                pl.semaphore_wait(barrier, 1)
            sends[t].start()

        for t, send in enumerate(sends):
            if t == num_tiles - 1:
                for finished in sends:
                    finished.wait_send()
            send.wait_recv()
            out_ref[:, pl.ds(t * _LANES, _LANES)] = mine[t] + theirs[t]

    out = pl.pallas_call(
        kernel_body,
        out_shape=jax.ShapeDtypeStruct((1, m), x.dtype),
        in_specs=[pl.BlockSpec(memory_space=pltpu.HBM)],
        out_specs=pl.BlockSpec(memory_space=pltpu.VMEM),
        scratch_shapes=[
            pltpu.VMEM((m, n), x.dtype),
            pltpu.VMEM((num_tiles, 1, _LANES), x.dtype),
            pltpu.VMEM((num_tiles, 1, _LANES), x.dtype),
            pltpu.SemaphoreType.DMA((num_copies,)),
            pltpu.SemaphoreType.DMA((num_tiles,)),
            pltpu.SemaphoreType.DMA((num_tiles,)),
        ],
        compiler_params=pltpu.CompilerParams(
            collective_id=0,
            disable_bounds_checks=True,
            disable_semaphore_checks=True,
            flags=_FLAGS,
        ),
    )(x)
    return out.reshape(m, 1)
```
